```python
import numpy as np

kernel_name = "dist_argmax_global_i_m4096_n1024"

def setup_inputs():
    return {"x": np.random.randn(16384, 1024).astype(np.float32)}

def reference(x: np.ndarray) -> np.ndarray:
    idx = np.argmax(x, axis=0).astype(np.float32)
    val = np.max(x, axis=0)
    return np.stack([val, idx], axis=0)
```

```python
import jax
import jax.numpy as jnp
from jax import lax
from jax.experimental import pallas as pl
from jax.experimental.pallas import tpu as pltpu

_M, _N = 4096, 1024
_NDEV = 4
_H = _N // 2
_NO_INDEX = 3e38

_PUSH = 192
_UNIT = 64
_CHUNK_UNITS = 4
_TAIL = ((128, 128), (128, 64, 32, 32))


def _scan(load, groups, best, bidx, ridx):
    for g in range(groups):
        v = load(g)
        keep = (v <= best) | (best != best)
        best = jnp.where(keep, best, v)
        bidx = jnp.where(keep, bidx, ridx)
        ridx = ridx + 8.0
    return best, bidx, ridx


def _reduce_sublanes(best, bidx):
    m = jnp.max(best, axis=0, keepdims=True)
    cand = (best == m) | (best != best)
    i = jnp.min(jnp.where(cand, bidx, jnp.float32(_NO_INDEX)), axis=0, keepdims=True)
    return m, i


def _combine(vals, idxs):
    vs = list(vals)
    while len(vs) > 1:
        vs = [jnp.maximum(vs[k], vs[k + 1]) for k in range(0, len(vs), 2)]
    m = vs[0]
    cs = [
        jnp.where((v == m) | (v != v), i, jnp.float32(_NO_INDEX))
        for v, i in zip(vals, idxs)
    ]
    while len(cs) > 1:
        cs = [jnp.minimum(cs[k], cs[k + 1]) for k in range(0, len(cs), 2)]
    return m, cs[0]


def pallas_dist_argmax_global_i_m4096_n1024_kernel(x: jax.Array):
    assert x.shape == (_M, _N) and x.dtype == jnp.float32, (x.shape, x.dtype)
    P, U = _PUSH, _UNIT
    tail = sum(_TAIL[0])
    L = _M - 2 * P
    La = L - tail
    nA = La // U
    CH = U * _CHUNK_UNITS
    nC = -(-La // CH)
    last_rows = La - (nC - 1) * CH
    blist = []
    for h, sizes in enumerate(_TAIL):
        r0 = La
        for sz in sizes:
            blist.append((h, r0, sz))
            r0 += sz

    def body(x_hbm, o_ref, buf, fbuf, fsbuf, sbuf, rbuf,
             a_sems, b_sems, push_ssem, push_rsem, fin_ssem, fin_rsems):
        me = lax.axis_index("i")
        right = (me + 1) % _NDEV
        left = (me + _NDEV - 1) % _NDEV

        def a_copy(c, rows=CH):
            r = pl.ds(c * CH if isinstance(c, int) else pl.multiple_of(c * CH, CH), rows)
            return pltpu.make_async_copy(x_hbm.at[r], buf.at[r], a_sems.at[c])

        def b_copy(k):
            h, r0, sz = blist[k]
            sl = (pl.ds(r0, sz), pl.ds(h * _H, _H))
            return pltpu.make_async_copy(x_hbm.at[sl], buf.at[sl], b_sems.at[k])

        for c in range(nC):
            a_copy(c, CH if c < nC - 1 else last_rows).start()
        for k in range(len(blist)):
            b_copy(k).start()

        bsem = pltpu.get_barrier_semaphore()
        for d in range(1, _NDEV):
            pl.semaphore_signal(bsem, inc=1, device_id=((me + d) % _NDEV,),
                                device_id_type=pl.DeviceIdType.MESH)
        pl.semaphore_wait(bsem, _NDEV - 1)

        for s, tgt in ((0, right), (1, left)):
            pltpu.make_async_remote_copy(
                x_hbm.at[pl.ds(L + s * P, P)], fbuf.at[s], push_ssem, push_rsem,
                device_id=(tgt,), device_id_type=pl.DeviceIdType.MESH).start()

        sub = lax.broadcasted_iota(jnp.int32, (8, _N), 0)
        ridx0 = (sub + me * _M).astype(jnp.float32)
        ninf = jnp.full((8, _N), -jnp.inf, jnp.float32)

        def unit(u, carry):
            @pl.when(jnp.logical_and(u % _CHUNK_UNITS == 0, u < (nC - 1) * _CHUNK_UNITS))
            def _():
                a_copy(u // _CHUNK_UNITS).wait()

            @pl.when(u == (nC - 1) * _CHUNK_UNITS)
            def _():
                a_copy(nC - 1, last_rows).wait()

            base = pl.multiple_of(u * U, U)
            return _scan(lambda g: buf[pl.ds(base + 8 * g, 8), :], U // 8, *carry)

        best, bidx, ridx = lax.fori_loop(0, nA, unit, (ninf, ridx0, ridx0))

        pltpu.make_async_copy(fbuf, fbuf, push_rsem).wait()
        swap = jnp.logical_or(me == 0, me == _NDEV - 1).astype(jnp.int32)
        nfu = P // U

        def funit(u, carry):
            fb, fi = carry
            seg = (u // nfu) ^ swap
            uu = u % nfu
            src_dev = jnp.where(seg == 0, left, right)
            row0 = src_dev * _M + L + seg * P + uu * U
            r0 = (sub + row0).astype(jnp.float32)
            base = pl.multiple_of(uu * U, U)
            fb, fi, _ = _scan(lambda g: fbuf[seg, pl.ds(base + 8 * g, 8), :], U // 8, fb, fi, r0)
            return fb, fi

        first_row = jnp.where(swap == 0, left * _M + L, right * _M + L + P)
        fi0 = (sub + first_row).astype(jnp.float32)
        fb, fi = lax.fori_loop(0, 2 * nfu, funit, (ninf, fi0))
        fm, fidx = _reduce_sublanes(fb, fi)
        fsbuf[0:1, :] = fm
        fsbuf[1:2, :] = fidx

        k = 0
        for h, sizes in enumerate(_TAIL):
            cols = slice(h * _H, (h + 1) * _H)
            bb, bi, rr = best[:, cols], bidx[:, cols], ridx[:, cols]
            for sz in sizes:
                r0 = blist[k][1]
                b_copy(k).wait()
                bb, bi, rr = _scan(lambda g: buf[pl.ds(r0 + 8 * g, 8), cols], sz // 8, bb, bi, rr)
                k += 1
            m, i = _reduce_sublanes(bb, bi)
            sbuf[0:1, cols] = m
            sbuf[1:2, cols] = i
            m, i = _combine([sbuf[0:1, cols], fsbuf[0:1, cols]],
                            [sbuf[1:2, cols], fsbuf[1:2, cols]])
            sbuf[0:1, cols] = m
            sbuf[1:2, cols] = i
            for d in (2, 1, 3):
                pltpu.make_async_remote_copy(
                    sbuf.at[:, cols], rbuf.at[d - 1, :, cols], fin_ssem, fin_rsems.at[h],
                    device_id=((me + d) % _NDEV,), device_id_type=pl.DeviceIdType.MESH).start()

        for h in range(2):
            cols = slice(h * _H, (h + 1) * _H)
            pltpu.make_async_copy(rbuf.at[:, :, cols], rbuf.at[:, :, cols], fin_rsems.at[h]).wait()
            m, i = _combine([sbuf[0:1, cols]] + [rbuf[d, 0:1, cols] for d in range(3)],
                            [sbuf[1:2, cols]] + [rbuf[d, 1:2, cols] for d in range(3)])
            o_ref[0:1, cols] = m
            o_ref[1:2, cols] = i

        pltpu.make_async_copy(rbuf, rbuf, fin_ssem).wait()
        pltpu.make_async_copy(fbuf, fbuf, push_ssem).wait()

    return pl.pallas_call(
        body,
        out_shape=jax.ShapeDtypeStruct((2, _N), jnp.float32),
        in_specs=[pl.BlockSpec(memory_space=pl.ANY)],
        out_specs=pl.BlockSpec(memory_space=pltpu.VMEM),
        scratch_shapes=[
            pltpu.VMEM((L, _N), jnp.float32),
            pltpu.VMEM((2, P, _N), jnp.float32),
            pltpu.VMEM((2, _N), jnp.float32),
            pltpu.VMEM((2, _N), jnp.float32),
            pltpu.VMEM((_NDEV - 1, 2, _N), jnp.float32),
            pltpu.SemaphoreType.DMA((nC,)),
            pltpu.SemaphoreType.DMA((len(blist),)),
            pltpu.SemaphoreType.DMA,
            pltpu.SemaphoreType.DMA,
            pltpu.SemaphoreType.DMA,
            pltpu.SemaphoreType.DMA((2,)),
        ],
        compiler_params=pltpu.CompilerParams(
            vmem_limit_bytes=48 * 1024 * 1024,
            collective_id=0,
            disable_semaphore_checks=True,
        ),
    )(x)
```

```python
import jax
import jax.numpy as jnp
from jax import lax
from jax.experimental import pallas as pl
from jax.experimental.pallas import tpu as pltpu

_M, _N = 4096, 1024
_NDEV = 4
_HALF = _N // 2
_NO_INDEX = 3e38

_PUSH = 208
_PUSH_UNIT = 104
_UNIT = 64
_CHUNK_UNITS = 4
_TAIL = ((144, 144), (160, 64, 32, 32))


def _scan(load, groups, best, bidx, ridx):
    for g in range(groups):
        v = load(g)
        keep = (v <= best) | (best != best)
        best = jnp.where(keep, best, v)
        bidx = jnp.where(keep, bidx, ridx)
        ridx = ridx + 8.0
    return best, bidx, ridx


def _index_if_max(v, i, m):
    return jnp.where((v == m) | (v != v), i, jnp.float32(_NO_INDEX))


def _tree(op, xs):
    xs = list(xs)
    while len(xs) > 1:
        xs = [op(xs[k], xs[k + 1]) for k in range(0, len(xs), 2)]
    return xs[0]


def pallas_dist_argmax_global_i_m4096_n1024_kernel(x: jax.Array):
    assert x.shape == (_M, _N) and x.dtype == jnp.float32, (x.shape, x.dtype)
    tail_rows = sum(_TAIL[0])
    assert sum(_TAIL[1]) == tail_rows
    local_rows = _M - 2 * _PUSH
    main_rows = local_rows - tail_rows
    assert main_rows % _UNIT == 0 and _PUSH % _PUSH_UNIT == 0
    n_units = main_rows // _UNIT
    chunk_rows = _UNIT * _CHUNK_UNITS
    n_chunks = pl.cdiv(main_rows, chunk_rows)
    last_chunk_rows = main_rows - (n_chunks - 1) * chunk_rows
    tail_chunks = []
    for h, sizes in enumerate(_TAIL):
        row = main_rows
        for size in sizes:
            tail_chunks.append((h, row, size))
            row += size

    def body(x_hbm, o_ref, buf, fbuf, sbuf, rbuf,
             main_sems, tail_sems, push_send, push_recv, part_send, part_recv):
        me = lax.axis_index("i")
        right = (me + 1) % _NDEV
        left = (me + _NDEV - 1) % _NDEV

        def main_copy(c, rows=chunk_rows):
            start = c * chunk_rows
            if not isinstance(c, int):
                start = pl.multiple_of(start, chunk_rows)
            r = pl.ds(start, rows)
            return pltpu.make_async_copy(x_hbm.at[r], buf.at[r], main_sems.at[c])

        def tail_copy(k):
            h, row, size = tail_chunks[k]
            r = (pl.ds(row, size), pl.ds(h * _HALF, _HALF))
            return pltpu.make_async_copy(x_hbm.at[r], buf.at[r], tail_sems.at[k])

        for c in range(2):
            main_copy(c).start()
        barrier = pltpu.get_barrier_semaphore()
        for d in (1, 3, 2):
            pl.semaphore_signal(barrier, inc=1, device_id=((me + d) % _NDEV,),
                                device_id_type=pl.DeviceIdType.MESH)
        for c in range(2, n_chunks):
            main_copy(c, chunk_rows if c < n_chunks - 1 else last_chunk_rows).start()
        for k in range(len(tail_chunks)):
            tail_copy(k).start()
        pl.semaphore_wait(barrier, _NDEV - 1)

        for s, target in ((0, right), (1, left)):
            pltpu.make_async_remote_copy(
                x_hbm.at[pl.ds(local_rows + s * _PUSH, _PUSH)], fbuf.at[s],
                push_send, push_recv,
                device_id=(target,), device_id_type=pl.DeviceIdType.MESH).start()

        sub = lax.broadcasted_iota(jnp.int32, (8, _N), 0)
        ninf = jnp.full((8, _N), -jnp.inf, jnp.float32)
        ridx0 = (sub + me * _M).astype(jnp.float32)

        def main_unit(u, carry):
            @pl.when(jnp.logical_and(u % _CHUNK_UNITS == 0,
                                     u < (n_chunks - 1) * _CHUNK_UNITS))
            def _():
                main_copy(u // _CHUNK_UNITS).wait()

            @pl.when(u == (n_chunks - 1) * _CHUNK_UNITS)
            def _():
                main_copy(n_chunks - 1, last_chunk_rows).wait()

            base = pl.multiple_of(u * _UNIT, _UNIT)
            return _scan(lambda g: buf[pl.ds(base + 8 * g, 8), :], _UNIT // 8, *carry)

        best, bidx, ridx = lax.fori_loop(0, n_units, main_unit, (ninf, ridx0, ridx0))

        pltpu.make_async_copy(fbuf, fbuf, push_recv).wait()
        swap = jnp.logical_or(me == 0, me == _NDEV - 1).astype(jnp.int32)

        def first_row(seg):
            return jnp.where(seg == 0, left * _M + local_rows,
                             right * _M + local_rows + _PUSH)

        def segment(t, carry):
            seg = t ^ swap
            r0 = (sub + first_row(seg)).astype(jnp.float32)

            def step(j, c):
                base = pl.multiple_of(j * _PUSH_UNIT, _PUSH_UNIT)
                return _scan(lambda g: fbuf[seg, pl.ds(base + 8 * g, 8), :],
                             _PUSH_UNIT // 8, *c)

            fb, fi, _ = lax.fori_loop(0, _PUSH // _PUSH_UNIT, step, (*carry, r0))
            return fb, fi

        fi0 = (sub + first_row(swap)).astype(jnp.float32)
        fb, fi = lax.fori_loop(0, 2, segment, (ninf, fi0))
        fm = jnp.max(fb, axis=0, keepdims=True)
        fidx = jnp.min(_index_if_max(fb, fi, fm), axis=0, keepdims=True)

        k = 0
        for h, sizes in enumerate(_TAIL):
            cols = slice(h * _HALF, (h + 1) * _HALF)
            b, bi, ri = best[:, cols], bidx[:, cols], ridx[:, cols]
            for size in sizes:
                row = tail_chunks[k][1]
                tail_copy(k).wait()
                b, bi, ri = _scan(lambda g: buf[pl.ds(row + 8 * g, 8), cols],
                                  size // 8, b, bi, ri)
                k += 1
            m = jnp.maximum(jnp.max(b, axis=0, keepdims=True), fm[:, cols])
            i = jnp.minimum(
                jnp.min(_index_if_max(b, bi, m), axis=0, keepdims=True),
                _index_if_max(fm[:, cols], fidx[:, cols], m))
            sbuf[0:1, cols] = m
            sbuf[1:2, cols] = i
            for d in (2, 1, 3):
                pltpu.make_async_remote_copy(
                    sbuf.at[:, cols], rbuf.at[d - 1, :, cols],
                    part_send, part_recv.at[h],
                    device_id=((me + d) % _NDEV,),
                    device_id_type=pl.DeviceIdType.MESH).start()

        def finish(h):
            cols = slice(h * _HALF, (h + 1) * _HALF)
            pltpu.make_async_copy(rbuf.at[:, :, cols], rbuf.at[:, :, cols],
                                  part_recv.at[h]).wait()
            vals = [sbuf[0:1, cols]] + [rbuf[d, 0:1, cols] for d in range(3)]
            idxs = [sbuf[1:2, cols]] + [rbuf[d, 1:2, cols] for d in range(3)]
            m = _tree(jnp.maximum, vals)
            o_ref[0:1, cols] = m
            o_ref[1:2, cols] = _tree(
                jnp.minimum, [_index_if_max(v, i, m) for v, i in zip(vals, idxs)])

        pltpu.make_async_copy(fbuf, fbuf, push_send).wait()
        finish(0)
        pltpu.make_async_copy(rbuf, rbuf, part_send).wait()
        finish(1)

    return pl.pallas_call(
        body,
        out_shape=jax.ShapeDtypeStruct((2, _N), jnp.float32),
        in_specs=[pl.BlockSpec(memory_space=pl.ANY)],
        out_specs=pl.BlockSpec(memory_space=pltpu.VMEM),
        scratch_shapes=[
            pltpu.VMEM((local_rows, _N), jnp.float32),
            pltpu.VMEM((2, _PUSH, _N), jnp.float32),
            pltpu.VMEM((2, _N), jnp.float32),
            pltpu.VMEM((_NDEV - 1, 2, _N), jnp.float32),
            pltpu.SemaphoreType.DMA((n_chunks,)),
            pltpu.SemaphoreType.DMA((len(tail_chunks),)),
            pltpu.SemaphoreType.DMA,
            pltpu.SemaphoreType.DMA,
            pltpu.SemaphoreType.DMA,
            pltpu.SemaphoreType.DMA((2,)),
        ],
        compiler_params=pltpu.CompilerParams(
            vmem_limit_bytes=48 * 1024 * 1024,
            collective_id=0,
            disable_semaphore_checks=True,
        ),
    )(x)
```

```python
import jax
import jax.numpy as jnp
from jax import lax
from jax.experimental import pallas as pl
from jax.experimental.pallas import tpu as pltpu

_M, _N = 4096, 1024
_NDEV = 4
_HALF = _N // 2
_NO_INDEX = 2**31 - 1
_INT_MIN = -(2**31)
_NAN_KEY = 0x7F800001

_PUSH = 208
_PUSH_UNIT = 104
_UNIT = 64
_CHUNK_UNITS = 4
_TAIL = ((144, 144), (160, 64, 32, 32))


def _to_key(v):
    b = lax.bitcast_convert_type(v, jnp.int32)
    signed = jnp.where(b < 0, jnp.int32(_INT_MIN) - b, b)
    return jnp.where(v != v, jnp.int32(_NAN_KEY), signed)


def _from_key(k):
    return lax.bitcast_convert_type(
        jnp.where(k < 0, jnp.int32(_INT_MIN) - k, k), jnp.float32)


def _scan(load, groups, best, bidx, ridx):
    for g in range(groups):
        k = _to_key(load(g))
        take = k > best
        best = jnp.where(take, k, best)
        bidx = jnp.where(take, ridx, bidx)
        ridx = ridx + 8
    return best, bidx, ridx


def _index_if_max(k, i, m):
    return jnp.where(k == m, i, jnp.int32(_NO_INDEX))


def _tree(op, xs):
    xs = list(xs)
    while len(xs) > 1:
        xs = [op(xs[k], xs[k + 1]) for k in range(0, len(xs), 2)]
    return xs[0]


def pallas_dist_argmax_global_i_m4096_n1024_kernel(x: jax.Array):
    assert x.shape == (_M, _N) and x.dtype == jnp.float32, (x.shape, x.dtype)
    tail_rows = sum(_TAIL[0])
    assert sum(_TAIL[1]) == tail_rows
    local_rows = _M - 2 * _PUSH
    main_rows = local_rows - tail_rows
    assert main_rows % _UNIT == 0 and _PUSH % _PUSH_UNIT == 0
    n_units = main_rows // _UNIT
    chunk_rows = _UNIT * _CHUNK_UNITS
    n_chunks = pl.cdiv(main_rows, chunk_rows)
    last_chunk_rows = main_rows - (n_chunks - 1) * chunk_rows
    tail_chunks = []
    for h, sizes in enumerate(_TAIL):
        row = main_rows
        for size in sizes:
            tail_chunks.append((h, row, size))
            row += size

    def body(x_hbm, o_ref, buf, fbuf, sbuf, rbuf,
             main_sems, tail_sems, push_send, push_recv, part_send, part_recv):
        me = lax.axis_index("i")
        right = (me + 1) % _NDEV
        left = (me + _NDEV - 1) % _NDEV

        def main_copy(c, rows=chunk_rows):
            start = c * chunk_rows
            if not isinstance(c, int):
                start = pl.multiple_of(start, chunk_rows)
            r = pl.ds(start, rows)
            return pltpu.make_async_copy(x_hbm.at[r], buf.at[r], main_sems.at[c])

        def tail_copy(k):
            h, row, size = tail_chunks[k]
            r = (pl.ds(row, size), pl.ds(h * _HALF, _HALF))
            return pltpu.make_async_copy(x_hbm.at[r], buf.at[r], tail_sems.at[k])

        for c in range(2):
            main_copy(c).start()
        barrier = pltpu.get_barrier_semaphore()
        for d in (1, 3, 2):
            pl.semaphore_signal(barrier, inc=1, device_id=((me + d) % _NDEV,),
                                device_id_type=pl.DeviceIdType.MESH)
        for c in range(2, n_chunks):
            main_copy(c, chunk_rows if c < n_chunks - 1 else last_chunk_rows).start()
        for k in range(len(tail_chunks)):
            tail_copy(k).start()
        pl.semaphore_wait(barrier, _NDEV - 1)

        for s, target in ((0, right), (1, left)):
            pltpu.make_async_remote_copy(
                x_hbm.at[pl.ds(local_rows + s * _PUSH, _PUSH)], fbuf.at[s],
                push_send, push_recv,
                device_id=(target,), device_id_type=pl.DeviceIdType.MESH).start()

        sub = lax.broadcasted_iota(jnp.int32, (8, _N), 0)
        lowest = jnp.full((8, _N), _INT_MIN, jnp.int32)
        ridx0 = sub + me * _M

        def main_unit(u, carry):
            @pl.when(jnp.logical_and(u % _CHUNK_UNITS == 0,
                                     u < (n_chunks - 1) * _CHUNK_UNITS))
            def _():
                main_copy(u // _CHUNK_UNITS).wait()

            @pl.when(u == (n_chunks - 1) * _CHUNK_UNITS)
            def _():
                main_copy(n_chunks - 1, last_chunk_rows).wait()

            base = pl.multiple_of(u * _UNIT, _UNIT)
            return _scan(lambda g: buf[pl.ds(base + 8 * g, 8), :], _UNIT // 8, *carry)

        best, bidx, ridx = lax.fori_loop(0, n_units, main_unit, (lowest, ridx0, ridx0))

        pltpu.make_async_copy(fbuf, fbuf, push_recv).wait()
        swap = jnp.logical_or(me == 0, me == _NDEV - 1).astype(jnp.int32)

        def first_row(seg):
            return jnp.where(seg == 0, left * _M + local_rows,
                             right * _M + local_rows + _PUSH)

        def segment(t, carry):
            seg = t ^ swap
            r0 = sub + first_row(seg)

            def step(j, c):
                base = pl.multiple_of(j * _PUSH_UNIT, _PUSH_UNIT)
                return _scan(lambda g: fbuf[seg, pl.ds(base + 8 * g, 8), :],
                             _PUSH_UNIT // 8, *c)

            fb, fi, _ = lax.fori_loop(0, _PUSH // _PUSH_UNIT, step, (*carry, r0))
            return fb, fi

        fi0 = sub + first_row(swap)
        fb, fi = lax.fori_loop(0, 2, segment, (lowest, fi0))
        fm = jnp.max(fb, axis=0, keepdims=True)
        fidx = jnp.min(_index_if_max(fb, fi, fm), axis=0, keepdims=True)

        k = 0
        for h, sizes in enumerate(_TAIL):
            cols = slice(h * _HALF, (h + 1) * _HALF)
            b, bi, ri = best[:, cols], bidx[:, cols], ridx[:, cols]
            for size in sizes:
                row = tail_chunks[k][1]
                tail_copy(k).wait()
                b, bi, ri = _scan(lambda g: buf[pl.ds(row + 8 * g, 8), cols],
                                  size // 8, b, bi, ri)
                k += 1
            m = jnp.maximum(jnp.max(b, axis=0, keepdims=True), fm[:, cols])
            i = jnp.minimum(
                jnp.min(_index_if_max(b, bi, m), axis=0, keepdims=True),
                _index_if_max(fm[:, cols], fidx[:, cols], m))
            sbuf[0:1, cols] = m
            sbuf[1:2, cols] = i
            for d in (2, 1, 3):
                pltpu.make_async_remote_copy(
                    sbuf.at[:, cols], rbuf.at[d - 1, :, cols],
                    part_send, part_recv.at[h],
                    device_id=((me + d) % _NDEV,),
                    device_id_type=pl.DeviceIdType.MESH).start()

        def finish(h):
            cols = slice(h * _HALF, (h + 1) * _HALF)
            pltpu.make_async_copy(rbuf.at[:, :, cols], rbuf.at[:, :, cols],
                                  part_recv.at[h]).wait()
            vals = [sbuf[0:1, cols]] + [rbuf[d, 0:1, cols] for d in range(3)]
            idxs = [sbuf[1:2, cols]] + [rbuf[d, 1:2, cols] for d in range(3)]
            m = _tree(jnp.maximum, vals)
            o_ref[0:1, cols] = _from_key(m)
            o_ref[1:2, cols] = _tree(
                jnp.minimum, [_index_if_max(v, i, m) for v, i in zip(vals, idxs)]
            ).astype(jnp.float32)

        pltpu.make_async_copy(fbuf, fbuf, push_send).wait()
        finish(0)
        pltpu.make_async_copy(rbuf, rbuf, part_send).wait()
        finish(1)

    return pl.pallas_call(
        body,
        out_shape=jax.ShapeDtypeStruct((2, _N), jnp.float32),
        in_specs=[pl.BlockSpec(memory_space=pl.ANY)],
        out_specs=pl.BlockSpec(memory_space=pltpu.VMEM),
        scratch_shapes=[
            pltpu.VMEM((local_rows, _N), jnp.float32),
            pltpu.VMEM((2, _PUSH, _N), jnp.float32),
            pltpu.VMEM((2, _N), jnp.int32),
            pltpu.VMEM((_NDEV - 1, 2, _N), jnp.int32),
            pltpu.SemaphoreType.DMA((n_chunks,)),
            pltpu.SemaphoreType.DMA((len(tail_chunks),)),
            pltpu.SemaphoreType.DMA,
            pltpu.SemaphoreType.DMA,
            pltpu.SemaphoreType.DMA,
            pltpu.SemaphoreType.DMA((2,)),
        ],
        compiler_params=pltpu.CompilerParams(
            vmem_limit_bytes=48 * 1024 * 1024,
            collective_id=0,
            disable_semaphore_checks=True,
        ),
    )(x)
```
